```python
import numpy as np

kernel_name = "dist_mlpseq_tp1d_rep_rep_b128_d128_h256"

def setup_inputs():
    x = np.random.randn(128, 128).astype(np.float32)
    Win0 = np.random.randn(128, 1024).astype(np.float32)
    Wout0 = np.random.randn(1024, 128).astype(np.float32)
    Win1 = np.random.randn(128, 1024).astype(np.float32)
    Wout1 = np.random.randn(1024, 128).astype(np.float32)
    Win2 = np.random.randn(128, 1024).astype(np.float32)
    Wout2 = np.random.randn(1024, 128).astype(np.float32)
    return {"x": x, "Win0": Win0, "Wout0": Wout0, "Win1": Win1, "Wout1": Wout1, "Win2": Win2, "Wout2": Wout2}

def reference(x, Win0, Win1, Win2, Wout0, Wout1, Wout2):
    h = x @ Win0
    h = np.maximum(h, 0.0)
    x = h @ Wout0
    h = x @ Win1
    h = np.maximum(h, 0.0)
    x = h @ Wout1
    h = x @ Win2
    h = np.maximum(h, 0.0)
    x = h @ Wout2
    return x
```

```python
import functools

import jax
import jax.numpy as jnp
from jax import lax
from jax.experimental import pallas as pl
from jax.experimental.pallas import tpu as pltpu

N_DEV = 4
N_LAYERS = 3
MESH = pl.DeviceIdType.MESH

SIZES = (16, 32, 32, 32, 16)
N_FIRST = 2

SCHEDULE = (
    (
        ' | d0 x0 y1 d1 | x1 d2 x2 d3 | x3 y0 d4 | y4 y2 x4 y3',
        'd0 y0 | d1 y1 | d2 y2 | y3 d3 x0 | y4 d4 x1 x2 x4 x3',
        ' | d1 d0 | x1 x0 y2 | x3 x2 | d2 y1 y3 y0 d3 x4 d4 y4',
    ),
    (
        'd0 d1 y1 y0 x1 |  | d2 y3 y2 x2 x0 d3 |  | x4 y4 x3 d4',
        'x0 d0 | d1 x1 y1 | x2 y0 d2 | d3 x3 | y3 d4 y2 x4 y4',
        'y0 | d1 y1 d0 | d2 y2 | x1 y3 | d4 x4 d3 x0 x2 x3 y4',
    ),
    (
        'd0 | d1 | y0 d2 y1 d3 y2 |  | x0 x1 y3 x3 d4 x2 x4 y4',
        'x0 d0 | d1 y0 x1 | d2 y1 x2 | d3 x3 y2 | y4 y3 d4 x4',
        'd0 | y0 d1 | d2 y1 | d3 | d4 y3 y4 x4 y2 x0 x3 x2 x1',
    ),
    (
        'd0 | d1 y1 x0 x1 y0 | y3 | d2 y4 d3 x3 y2 x2 x4 | d4',
        'd0 | d1 y0 y1 x1 | d2 y2 | d3 | d4 x0 x2 x4 y3 x3 y4',
        ' | y1 d1 x1 y0 | x0 x2 | x3 | x4 d4 y4 d0 y2 y3 d2 d3',
    ),
)

_KINDS = "dxy"
N_CHUNKS = len(SIZES)
OFFS = tuple(sum(SIZES[:c]) for c in range(N_CHUNKS))


def _parse(text):
    return tuple(
        tuple((int(tok[1:]), _KINDS.index(tok[0])) for tok in group.split())
        for group in text.split("|")
    )


TABLES = tuple(tuple(_parse(t) for t in per_chip) for per_chip in SCHEDULE)


def _validate():
    every = sorted((c, k) for c in range(N_CHUNKS) for k in range(N_DEV - 1))
    for per_chip in TABLES:
        for layer, table in enumerate(per_chip):
            assert len(table) == N_CHUNKS
            assert sorted(m for group in table for m in group) == every
            for step, group in enumerate(table):
                for c, _ in group:
                    if layer == 0:
                        assert c < N_FIRST or step >= N_FIRST
                    else:
                        assert c <= step


_validate()


def pallas_dist_mlpseq_tp1d_rep_rep_b128_d128_h256_kernel(
    x: jax.Array,
    Win0: jax.Array,
    Wout0: jax.Array,
    Win1: jax.Array,
    Wout1: jax.Array,
    Win2: jax.Array,
    Wout2: jax.Array,
):
    B, D = x.shape
    H = Win0.shape[1]
    assert B == sum(SIZES) and H == 2 * D
    bf16, f32 = jnp.bfloat16, jnp.float32
    r0 = sum(SIZES[:N_FIRST])

    def body(x_hbm, win0, wout0, win1, wout1, win2, wout2, out_ref,
             xv, winv, woutv, sbuf, rbuf, in_sems, send_sem, recv_sems):
        me = lax.axis_index("i")
        peers = (me ^ 2, 3 - me, me ^ 1)
        barrier = pltpu.get_barrier_semaphore()

        wins = (win0, win1, win2)
        wouts = (wout0, wout1, wout2)
        load_x0 = pltpu.make_async_copy(
            x_hbm.at[pl.ds(0, r0)], xv.at[pl.ds(0, r0)], in_sems.at[0])
        load_x1 = pltpu.make_async_copy(
            x_hbm.at[pl.ds(r0, B - r0)], xv.at[pl.ds(r0, B - r0)], in_sems.at[1])
        load_win = [pltpu.make_async_copy(wins[l], winv.at[l], in_sems.at[2 + 2 * l])
                    for l in range(N_LAYERS)]
        load_wout = [pltpu.make_async_copy(wouts[l], woutv.at[l], in_sems.at[3 + 2 * l])
                     for l in range(N_LAYERS)]
        load_x0.start()
        load_win[0].start()
        load_wout[0].start()
        load_x1.start()
        for peer in peers:
            pl.semaphore_signal(barrier, inc=1, device_id=(peer,), device_id_type=MESH)

        def start_copies(layer, group):
            for c, k in group:
                rows = pl.ds(OFFS[c], SIZES[c])
                pltpu.make_async_remote_copy(
                    src_ref=sbuf.at[layer, rows],
                    dst_ref=rbuf.at[layer, k, rows],
                    send_sem=send_sem,
                    recv_sem=recv_sems.at[layer, c],
                    device_id=(peers[k],),
                    device_id_type=MESH,
                ).start()

        def send(layer, step):
            for p in range(N_DEV):
                group = TABLES[p][layer][step]
                if group:
                    pl.when(me == p)(functools.partial(start_copies, layer, group))

        def all_reduced(own, layer, c):
            rows = pl.ds(OFFS[c], SIZES[c])
            landed = rbuf.at[layer, :, rows]
            pltpu.make_async_copy(landed, landed, recv_sems.at[layer, c]).wait()
            r = [rbuf[layer, k, rows, :].astype(f32) for k in range(N_DEV - 1)]
            return (own + r[0]) + (r[1] + r[2])

        def halves_in(l):
            return [winv[l, :, i * D:(i + 1) * D].astype(bf16) for i in range(2)]

        def halves_out(l):
            return [woutv[l, i * D:(i + 1) * D, :].astype(bf16) for i in range(2)]

        def hidden(s, w):
            s = s.astype(bf16)
            return [jnp.maximum(jnp.dot(s, wi, preferred_element_type=f32), 0.0).astype(bf16)
                    for wi in w]

        def project(h, wo):
            return (jnp.dot(h[0], wo[0], preferred_element_type=f32)
                    + jnp.dot(h[1], wo[1], preferred_element_type=f32))

        load_x0.wait()
        load_win[0].wait()
        w = halves_in(0)
        h_first = hidden(xv[0:r0, :], w)
        load_wout[0].wait()
        wo = halves_out(0)
        p_first = project(h_first, wo)
        sbuf[0, 0:r0, :] = p_first.astype(bf16)
        pl.semaphore_wait(barrier, N_DEV - 1)
        for c in range(N_FIRST):
            send(0, c)
        load_x1.wait()
        p_rest = project(hidden(xv[r0:B, :], w), wo)
        sbuf[0, r0:B, :] = p_rest.astype(bf16)
        for c in range(N_FIRST, N_CHUNKS):
            send(0, c)
        own = [p_first[OFFS[c]:OFFS[c] + SIZES[c]] if c < N_FIRST
               else p_rest[OFFS[c] - r0:OFFS[c] - r0 + SIZES[c]]
               for c in range(N_CHUNKS)]
        for l in range(1, N_LAYERS):
            load_win[l].start()
            load_wout[l].start()

        for l in range(1, N_LAYERS):
            load_win[l].wait()
            load_wout[l].wait()
            w = halves_in(l)
            wo = halves_out(l)
            for c in range(N_CHUNKS):
                p = project(hidden(all_reduced(own[c], l - 1, c), w), wo)
                sbuf[l, pl.ds(OFFS[c], SIZES[c]), :] = p.astype(bf16)
                send(l, c)
                own[c] = p

        for c in range(N_CHUNKS):
            out_ref[pl.ds(OFFS[c], SIZES[c]), :] = all_reduced(own[c], N_LAYERS - 1, c)
        pltpu.make_async_copy(rbuf, rbuf, send_sem).wait()

    return pl.pallas_call(
        body,
        out_shape=jax.ShapeDtypeStruct((B, D), f32),
        in_specs=[pl.BlockSpec(memory_space=pl.ANY)] * 7,
        out_specs=pl.BlockSpec(memory_space=pltpu.VMEM),
        scratch_shapes=[
            pltpu.VMEM((B, D), f32),
            pltpu.VMEM((N_LAYERS, D, H), f32),
            pltpu.VMEM((N_LAYERS, H, D), f32),
            pltpu.VMEM((N_LAYERS, B, D), bf16),
            pltpu.VMEM((N_LAYERS, N_DEV - 1, B, D), bf16),
            pltpu.SemaphoreType.DMA((2 + 2 * N_LAYERS,)),
            pltpu.SemaphoreType.DMA,
            pltpu.SemaphoreType.DMA((N_LAYERS, N_CHUNKS)),
        ],
        compiler_params=pltpu.CompilerParams(
            collective_id=0,
            disable_semaphore_checks=True,
            disable_bounds_checks=True,
        ),
    )(x, Win0, Wout0, Win1, Wout1, Win2, Wout2)
```

```python
import functools

import jax
import jax.numpy as jnp
from jax import lax
from jax.experimental import pallas as pl
from jax.experimental.pallas import tpu as pltpu

N_DEV = 4
N_LAYERS = 3
MESH = pl.DeviceIdType.MESH

SIZES = (16, 16, 16, 16, 16, 16, 16, 16)
N_FIRST = 3

SCHEDULE = (
    (
        'd0 y0 x0 | d1 | x1 |  | x2 d2 y5 y1 d3 | y2 y3 y4 x3 d4 y6 d5 x4 | x5 y7 x6 | d6 d7 x7',
        'd0 | y0 d1 x0 y1 | d2 y2 | d3 | d4 y4 | d5 y5 | d6 x5 | x1 d7 y3 x2 x3 y7 x4 x7 x6 y6',
        ' |  | d1 | x0 y1 d2 x3 y2 | d0 d3 x1 | y3 x4 x5 | y4 d4 y5 y6 d6 | d7 y7 d5 x6 y0 x7 x2',
    ),
    (
        ' | d0 y2 y0 d1 y1 | x0 d2 | x4 d3 x3 | x5 d4 y6 d5 | d6 x2 x1 | d7 y7 y5 y4 x6 y3 x7 | ',
        'd0 | x0 d1 | d2 x2 | y0 x1 y1 d3 x3 | d4 | y2 | x4 x6 y6 d5 y5 x5 d6 | d7 x7 y7 y3 y4',
        'y0 | y1 | y2 | y3 | y4 x4 d0 d3 d4 d2 | x3 y5 d5 | y6 x6 d6 | d7 x2 d1 x0 x5 x1 y7 x7',
    ),
    (
        'd0 y2 |  | d1 y0 d2 |  | d3 d4 | x0 d5 d6 | x1 d7 y3 | x3 y1 y4 x2 x4 y5 y6 x5 y7 x7 x6',
        'x0 | d0 x1 d1 | x2 y2 y1 d2 | y0 x3 d3 | x4 y4 | d5 y3 d4 x5 | y5 d6 | x6 y6 x7 y7 d7',
        'd0 y0 | d1 | d2 | d3 | d4 x1 | d5 | y3 d6 | y7 d7 x3 x6 y2 x2 x7 x4 y4 y6 y5 y1 x5 x0',
    ),
    (
        ' |  | d1 d0 x0 y2 |  | x5 d3 d2 y4 x1 d4 y3 x2 | d5 x4 | y6 x3 d6 y7 x7 x6 y0 d7 y5 | y1',
        'y0 d0 | d1 | d2 y1 y2 | d3 y3 | d4 | y5 d5 x4 | x1 d6 | x0 d7 y4 x6 y6 x2 x3 y7 x5 x7',
        ' | y1 d0 x0 |  | x1 x2 y2 x3 | d4 x4 y3 | x5 | x6 y6 | y0 x7 d7 d3 y4 d5 y5 d2 y7 d6 d1',
    ),
)

OVERLAP = (
    ('11111100', '01101000'),
    ('10111100', '11001000'),
    ('10110010', '10101110'),
    ('01001010', '11111010'),
)

_KINDS = "dxy"
N_CHUNKS = len(SIZES)
OFFS = tuple(sum(SIZES[:c]) for c in range(N_CHUNKS))


def _parse(text):
    return tuple(
        tuple((int(tok[1:]), _KINDS.index(tok[0])) for tok in group.split())
        for group in text.split("|")
    )


TABLES = tuple(tuple(_parse(t) for t in per_chip) for per_chip in SCHEDULE)


def _validate():
    every = sorted((c, k) for c in range(N_CHUNKS) for k in range(N_DEV - 1))
    for per_chip in TABLES:
        for layer, table in enumerate(per_chip):
            assert len(table) == N_CHUNKS
            assert sorted(m for group in table for m in group) == every
            for step, group in enumerate(table):
                for c, _ in group:
                    if layer == 0:
                        assert c < N_FIRST or step >= N_FIRST
                    else:
                        assert c <= step


_validate()


def pallas_dist_mlpseq_tp1d_rep_rep_b128_d128_h256_kernel(
    x: jax.Array,
    Win0: jax.Array,
    Wout0: jax.Array,
    Win1: jax.Array,
    Wout1: jax.Array,
    Win2: jax.Array,
    Wout2: jax.Array,
):
    B, D = x.shape
    H = Win0.shape[1]
    assert B == sum(SIZES) and H == 2 * D
    bf16, f32 = jnp.bfloat16, jnp.float32
    r0 = sum(SIZES[:N_FIRST])

    def body(x_hbm, win0, wout0, win1, wout1, win2, wout2, out_ref,
             xv, winv, woutv, sbuf, rbuf, in_sems, send_sem, recv_sems):
        me = lax.axis_index("i")
        barrier = pltpu.get_barrier_semaphore()

        wins = (win0, win1, win2)
        wouts = (wout0, wout1, wout2)
        load_x0 = pltpu.make_async_copy(
            x_hbm.at[pl.ds(0, r0)], xv.at[pl.ds(0, r0)], in_sems.at[0])
        load_x1 = pltpu.make_async_copy(
            x_hbm.at[pl.ds(r0, B - r0)], xv.at[pl.ds(r0, B - r0)], in_sems.at[1])
        load_win = [pltpu.make_async_copy(wins[l], winv.at[l], in_sems.at[2 + 2 * l])
                    for l in range(N_LAYERS)]
        load_wout = [pltpu.make_async_copy(wouts[l], woutv.at[l], in_sems.at[3 + 2 * l])
                     for l in range(N_LAYERS)]
        load_x0.start()
        load_win[0].start()
        load_wout[0].start()
        load_x1.start()
        for peer in (me ^ 2, 3 - me, me ^ 1):
            pl.semaphore_signal(barrier, inc=1, device_id=(peer,), device_id_type=MESH)

        def halves_in(l):
            return [winv[l, :, i * D:(i + 1) * D].astype(bf16) for i in range(2)]

        def halves_out(l):
            return [woutv[l, i * D:(i + 1) * D, :].astype(bf16) for i in range(2)]

        def hidden(s, w):
            s = s.astype(bf16)
            return [jnp.maximum(jnp.dot(s, wi, preferred_element_type=f32), 0.0).astype(bf16)
                    for wi in w]

        def project(h, wo):
            return (jnp.dot(h[0], wo[0], preferred_element_type=f32)
                    + jnp.dot(h[1], wo[1], preferred_element_type=f32))

        def run(pos):
            peers = (pos ^ 2, 3 - pos, pos ^ 1)

            def send(layer, step):
                for c, k in TABLES[pos][layer][step]:
                    rows = pl.ds(OFFS[c], SIZES[c])
                    pltpu.make_async_remote_copy(
                        src_ref=sbuf.at[layer, rows],
                        dst_ref=rbuf.at[layer, k, rows],
                        send_sem=send_sem,
                        recv_sem=recv_sems.at[layer, c],
                        device_id=(peers[k],),
                        device_id_type=MESH,
                    ).start()

            def all_reduced(own, layer, c):
                rows = pl.ds(OFFS[c], SIZES[c])
                landed = rbuf.at[layer, :, rows]
                pltpu.make_async_copy(landed, landed, recv_sems.at[layer, c]).wait()
                r = [rbuf[layer, k, rows, :].astype(f32) for k in range(N_DEV - 1)]
                return (own + r[0]) + (r[1] + r[2])

            load_x0.wait()
            load_win[0].wait()
            w = halves_in(0)
            h_first = hidden(xv[0:r0, :], w)
            load_wout[0].wait()
            wo = halves_out(0)
            p_first = project(h_first, wo)
            sbuf[0, 0:r0, :] = p_first.astype(bf16)
            pl.semaphore_wait(barrier, N_DEV - 1)
            for c in range(N_FIRST):
                send(0, c)
            load_x1.wait()
            p_rest = project(hidden(xv[r0:B, :], w), wo)
            sbuf[0, r0:B, :] = p_rest.astype(bf16)
            for c in range(N_FIRST, N_CHUNKS):
                send(0, c)
            own = [p_first[OFFS[c]:OFFS[c] + SIZES[c]] if c < N_FIRST
                   else p_rest[OFFS[c] - r0:OFFS[c] - r0 + SIZES[c]]
                   for c in range(N_CHUNKS)]
            for l in range(1, N_LAYERS):
                load_win[l].start()
                load_wout[l].start()

            for l in range(1, N_LAYERS):
                load_win[l].wait()
                load_wout[l].wait()
                w = halves_in(l)
                wo = halves_out(l)

                def finish(c, h):
                    p = project(h, wo)
                    sbuf[l, pl.ds(OFFS[c], SIZES[c]), :] = p.astype(bf16)
                    send(l, c)
                    own[c] = p

                pending = None
                for c in range(N_CHUNKS):
                    s = all_reduced(own[c], l - 1, c)
                    if pending is not None:
                        finish(*pending)
                        pending = None
                    h = hidden(s, w)
                    if OVERLAP[pos][l - 1][c] == "1":
                        pending = (c, h)
                    else:
                        finish(c, h)
                assert pending is None

            for c in range(N_CHUNKS):
                out_ref[pl.ds(OFFS[c], SIZES[c]), :] = all_reduced(own[c], N_LAYERS - 1, c)
            pltpu.make_async_copy(rbuf, rbuf, send_sem).wait()

        for pos in range(N_DEV):
            pl.when(me == pos)(functools.partial(run, pos))

    return pl.pallas_call(
        body,
        out_shape=jax.ShapeDtypeStruct((B, D), f32),
        in_specs=[pl.BlockSpec(memory_space=pl.ANY)] * 7,
        out_specs=pl.BlockSpec(memory_space=pltpu.VMEM),
        scratch_shapes=[
            pltpu.VMEM((B, D), f32),
            pltpu.VMEM((N_LAYERS, D, H), f32),
            pltpu.VMEM((N_LAYERS, H, D), f32),
            pltpu.VMEM((N_LAYERS, B, D), bf16),
            pltpu.VMEM((N_LAYERS, N_DEV - 1, B, D), bf16),
            pltpu.SemaphoreType.DMA((2 + 2 * N_LAYERS,)),
            pltpu.SemaphoreType.DMA,
            pltpu.SemaphoreType.DMA((N_LAYERS, N_CHUNKS)),
        ],
        compiler_params=pltpu.CompilerParams(
            collective_id=0,
            disable_semaphore_checks=True,
            disable_bounds_checks=True,
        ),
    )(x, Win0, Wout0, Win1, Wout1, Win2, Wout2)
```
